```python
import numpy as np

kernel_name = "dist_ar_xy_y_m256_n256"

def setup_inputs():
    return {"x": np.random.randn(512, 256).astype(np.float32)}

def reference(x: np.ndarray) -> np.ndarray:
    return x.reshape(2, 256, 256).sum(axis=0)
```

```python
import jax
import jax.numpy as jnp
from jax import lax
from jax.experimental import pallas as pl
from jax.experimental.pallas import tpu as pltpu


def pallas_dist_ar_xy_y_m256_n256_kernel(x: jax.Array):
    m, n = x.shape

    def body(x_ref, o_ref, send_buf, recv_buf, send_sem, recv_sem):
        my_x = lax.axis_index("x")
        my_y = lax.axis_index("y")
        peer = (my_x, 1 - my_y)
        barrier = pltpu.get_barrier_semaphore()
        pl.semaphore_signal(barrier, inc=1, device_id=peer,
                            device_id_type=pl.DeviceIdType.MESH)
        send_buf[...] = x_ref[...].astype(jnp.bfloat16)
        pl.semaphore_wait(barrier, 1)
        rdma = pltpu.make_async_remote_copy(
            src_ref=send_buf, dst_ref=recv_buf, send_sem=send_sem, recv_sem=recv_sem,
            device_id=peer, device_id_type=pl.DeviceIdType.MESH)
        rdma.start()
        rdma.wait_recv()
        o_ref[...] = x_ref[...] + recv_buf[...].astype(jnp.float32)
        rdma.wait_send()

    return pl.pallas_call(
        body,
        out_shape=jax.ShapeDtypeStruct((m, n), x.dtype),
        in_specs=[pl.BlockSpec(memory_space=pltpu.VMEM)],
        out_specs=pl.BlockSpec(memory_space=pltpu.VMEM),
        scratch_shapes=[
            pltpu.VMEM((m, n), jnp.bfloat16),
            pltpu.VMEM((m, n), jnp.bfloat16),
            pltpu.SemaphoreType.DMA,
            pltpu.SemaphoreType.DMA,
        ],
        compiler_params=pltpu.CompilerParams(collective_id=0),
    )(x)
```

```python
import jax
import jax.numpy as jnp
from jax import lax
from jax.experimental import pallas as pl
from jax.experimental.pallas import tpu as pltpu

_D00, _D01, _D10, _D11 = 0, 1, 2, 3

_N_QUARTERS = 128
_F_END = 25
_F_HEAD = 4
_C_HEAD = 6
_C_SIZES = (4, 8, 20)
_C_TAIL = 4
_G_SIZE = 12
_A_SPLIT = 48


def _rows(r0, r1):
    return (r0, r1 - r0, 0, 256)


def _cover(q0, q1):
    pieces = []
    while q0 < q1:
        row, col = 8 * (q0 // 4), 128 * (q0 // 2 % 2)
        if q0 % 4 == 0 and q1 - q0 >= 4:
            n = (q1 - q0) // 4
            pieces.append((row, 8 * n, 0, 256))
            q0 += 4 * n
        elif q0 % 2 == 0 and q1 - q0 >= 2:
            pieces.append((row, 8, col, 128))
            q0 += 2
        else:
            pieces.append((row + 4 * (q0 % 2), 4, col, 128))
            q0 += 1
    return pieces


def _tiles(q0, q1):
    return _cover(q0 - q0 % 2, q1 + q1 % 2)


def _c_chunks():
    q = _F_END + _C_HEAD
    ends = [q + -q % 4] if q % 4 else []
    for size in _C_SIZES:
        ends.append((ends[-1] if ends else q) + size)
    ends += [_N_QUARTERS - _C_TAIL, _N_QUARTERS]
    return list(zip([q] + ends[:-1], ends))


_G_START = _F_END + _C_HEAD + -(_F_END + _C_HEAD) % 4
_G = _rows(2 * _G_START, 2 * (_G_START + _G_SIZE))
_F_PIECES = [_cover(q, q + 1)[0] for q in range(_F_END)]
_C_HEAD_PIECES = _cover(_F_END, _F_END + _C_HEAD)
_C_CHUNKS = _c_chunks()
_R_PIECES = _cover(_F_END, _G_START) + _cover(_G_START + _G_SIZE, _N_QUARTERS)
_N_COPIES = (
    2 * len(_F_PIECES)
    + len(_C_HEAD_PIECES)
    + sum(len(_cover(*c)) for c in _C_CHUNKS)
    + len(_R_PIECES)
    + 5
)
_N_LOADS = 12


def _body(x_hbm, o_ref, own, own16, got32, got16, load_sems, send_sems, recv_sems):
    barrier = pltpu.get_barrier_semaphore()

    def at(piece):
        r0, rows, c0, cols = piece
        return pl.ds(r0, rows), pl.ds(c0, cols)

    n_copies = 0

    def remote(src, dst, piece, target):
        nonlocal n_copies
        i, n_copies = n_copies, n_copies + 1
        return lambda: pltpu.make_async_remote_copy(
            src.at[at(piece)],
            dst.at[at(piece)],
            send_sems.at[i],
            recv_sems.at[i],
            device_id=target,
            device_id_type=pl.DeviceIdType.LOGICAL,
        )

    def start_loads(pieces):
        loads = [
            pltpu.make_async_copy(x_hbm.at[at(p)], own.at[at(p)], load_sems.at[i])
            for i, p in enumerate(pieces)
        ]
        for load in loads:
            load.start()
        return loads

    def signal(target):
        pl.semaphore_signal(
            barrier, inc=1, device_id=target, device_id_type=pl.DeviceIdType.LOGICAL
        )

    def round_own(piece):
        own16[at(piece)] = own[at(piece)].astype(jnp.bfloat16)

    def add(got, piece):
        o_ref[at(piece)] = own[at(piece)] + got[at(piece)].astype(jnp.float32)

    f_got = [got32 if q < _F_HEAD else got16 for q in range(_F_END)]
    f_src = [x_hbm if q < _F_HEAD else own16 for q in range(_F_END)]
    f_in = [remote(s, g, p, _D10) for s, g, p in zip(f_src, f_got, _F_PIECES)]
    f_on = [remote(g, g, p, _D00) for g, p in zip(f_got, _F_PIECES)]
    c_head = [remote(x_hbm, got32, p, _D00) for p in _C_HEAD_PIECES]
    c_rest = [
        [(p, remote(own16, got16, p, _D00)) for p in _cover(*chunk)]
        for chunk in _C_CHUNKS
    ]
    r_rest = [remote(own16, got16, p, _D10) for p in _R_PIECES]
    g_on = remote(got16, got16, _G, _D10)
    a_low, a_high = _rows(0, _A_SPLIT), _rows(_A_SPLIT, 256)
    a_low_in = remote(own16, got16, a_low, _D11)
    a_low_on = remote(got16, got16, a_low, _D01)
    a_high_11 = remote(own16, got16, a_high, _D11)
    a_high_01 = remote(own16, got16, a_high, _D01)
    assert n_copies == _N_COPIES

    def chip_01():
        signal(_D11)
        pl.semaphore_wait(barrier, 1)
        for copy in c_head:
            copy().start()
        first = _C_CHUNKS[0][0]
        tiles = [_tiles(*chunk) for chunk in _C_CHUNKS]
        loads = start_loads(sum(tiles, []) + _cover(0, first - first % 2))
        signal(_D00)
        for needed, copies in zip(tiles, c_rest):
            for piece in needed:
                loads.pop(0).wait()
                round_own(piece)
            for _, copy in copies:
                copy().start()
        for load in loads:
            load.wait()
        for copy in c_head + [copy for copies in c_rest for _, copy in copies]:
            copy().wait_send()
        a_low_on().wait_recv()
        add(got16, a_low)
        a_high_01().wait_recv()
        add(got16, a_high)

    def chip_10():
        signal(_D11)
        signal(_D00)
        (load,) = start_loads([_rows(0, 256)])
        load.wait()
        round_own(_rows(0, 256))
        pl.semaphore_wait(barrier, 2)
        a_low_in().start()
        a_high_11().start()
        for arrived, onward in zip(f_in, f_on):
            arrived().wait_recv()
            onward().start()
        for piece in _cover(0, _F_HEAD):
            add(got32, piece)
        for piece in _cover(_F_HEAD, _F_END):
            add(got16, piece)
        g_on().wait_recv()
        add(got16, _G)
        for copy in f_on + [a_low_in, a_high_11]:
            copy().wait_send()
        for piece, copy in zip(_R_PIECES, r_rest):
            copy().wait_recv()
            add(got16, piece)

    def chip_11():
        signal(_D10)
        f_rows = 2 * (_F_END + -_F_END % 4)
        head_rows = 2 * _F_HEAD
        first, second = _rows(head_rows, head_rows + 8), _rows(head_rows + 8, f_rows)
        loads = start_loads([first, second, _rows(f_rows, 256), _rows(0, head_rows)])
        pl.semaphore_wait(barrier, 2)
        for copy in f_in[:_F_HEAD]:
            copy().start()
        loads[0].wait()
        round_own(first)
        for copy in f_in[_F_HEAD : _F_HEAD + 4]:
            copy().start()
        loads[1].wait()
        round_own(second)
        for copy in f_in[_F_HEAD + 4 :]:
            copy().start()
        loads[2].wait()
        round_own(_rows(f_rows, 256))
        for copy in r_rest:
            copy().start()
        loads[3].wait()
        a_low_in().wait_recv()
        a_low_on().start()
        add(got16, a_low)
        for copy in f_in + r_rest + [a_low_on]:
            copy().wait_send()
        a_high_11().wait_recv()
        add(got16, a_high)

    def chip_00():
        signal(_D01)
        signal(_D10)
        (load,) = start_loads([_rows(0, 256)])
        load.wait()
        round_own(a_high)
        pl.semaphore_wait(barrier, 2)
        a_high_01().start()
        for piece, copy in zip(_C_HEAD_PIECES, c_head):
            copy().wait_recv()
            add(got32, piece)
        passed_on = False
        for (_, end), copies in zip(_C_CHUNKS[:-2], c_rest):
            for piece, copy in copies:
                copy().wait_recv()
            if not passed_on and end >= _G_START + _G_SIZE:
                g_on().start()
                passed_on = True
            for piece, _ in copies:
                add(got16, piece)
        assert passed_on
        a_high_01().wait_send()
        g_on().wait_send()
        last = list(zip(f_got, _F_PIECES, f_on))
        order = (
            last[:-2]
            + [(got16, *c) for c in c_rest[-2]]
            + last[-2:-1]
            + [(got16, *c) for c in c_rest[-1]]
            + last[-1:]
        )
        for got, piece, copy in order:
            copy().wait_recv()
            add(got, piece)

    me = 2 * lax.axis_index("x") + lax.axis_index("y")
    pl.when(me == _D01)(chip_01)
    pl.when(me == _D10)(chip_10)
    pl.when(me == _D11)(chip_11)
    pl.when(me == _D00)(chip_00)


def pallas_dist_ar_xy_y_m256_n256_kernel(x: jax.Array):
    assert x.shape == (256, 256) and x.dtype == jnp.float32
    return pl.pallas_call(
        _body,
        out_shape=jax.ShapeDtypeStruct(x.shape, x.dtype),
        in_specs=[pl.BlockSpec(memory_space=pltpu.HBM)],
        out_specs=pl.BlockSpec(memory_space=pltpu.VMEM),
        scratch_shapes=[
            pltpu.VMEM(x.shape, jnp.float32),
            pltpu.VMEM(x.shape, jnp.bfloat16),
            pltpu.VMEM(x.shape, jnp.float32),
            pltpu.VMEM(x.shape, jnp.bfloat16),
            pltpu.SemaphoreType.DMA((_N_LOADS,)),
            pltpu.SemaphoreType.DMA((_N_COPIES,)),
            pltpu.SemaphoreType.DMA((_N_COPIES,)),
        ],
        compiler_params=pltpu.CompilerParams(
            collective_id=0,
            disable_semaphore_checks=True,
        ),
    )(x)
```

```python
import jax
import jax.numpy as jnp
from jax import lax
from jax.experimental import pallas as pl
from jax.experimental.pallas import tpu as pltpu

_D00, _D01, _D10, _D11 = 0, 1, 2, 3


def _rows(start, stop):
    return (start, stop - start, 0, 256)


def _tile(t):
    return (8 * (t // 2), 8, 128 * (t % 2), 128)


def _strips(tile):
    row, rows, col, cols = tile
    return [(r, 2, col, cols) for r in range(row, row + rows, 2)]


_F_HEAD = [_tile(0), _tile(1)]
_F_GROUPS = [
    (_tile(2), [_tile(2)]),
    (_tile(3), [_tile(3)]),
    (_rows(16, 24), [_tile(4), _tile(5)]),
    (_rows(24, 56), [_tile(t) for t in range(6, 13)]),
]
_F_REST = [tile for _, tiles in _F_GROUPS for tile in tiles]
_C_HEAD = [_tile(13), _rows(56, 64)]
_C_REST = [
    _tile(16),
    _tile(17),
    _rows(72, 80),
    _rows(80, 96),
    _rows(96, 128),
    _rows(128, 248),
    _rows(248, 256),
]
_G = _rows(64, 88)
_G_READY = 4
_R_EARLY = [_tile(13), _rows(56, 64), _rows(88, 120)]
_R_LATE = _rows(120, 256)
_A_LOW, _A_HIGH = _rows(0, 48), _rows(48, 256)

_N_LOADS = len(_C_REST) + 1
_N_COPIES = (
    8 * (len(_F_HEAD) + len(_F_REST)) + len(_C_HEAD) + len(_C_REST) + len(_R_EARLY) + 6
)


def _body(x_hbm, o_ref, own, own16, got32, got16, load_sems, send_sems, recv_sems):
    barrier = pltpu.get_barrier_semaphore()

    def at(piece):
        row, rows, col, cols = piece
        return pl.ds(row, rows), pl.ds(col, cols)

    n_copies = 0

    def remote(src, dst, piece, target):
        nonlocal n_copies
        i, n_copies = n_copies, n_copies + 1
        return lambda: pltpu.make_async_remote_copy(
            src.at[at(piece)],
            dst.at[at(piece)],
            send_sems.at[i],
            recv_sems.at[i],
            device_id=target,
            device_id_type=pl.DeviceIdType.LOGICAL,
        )

    def start_load(i, piece):
        load = pltpu.make_async_copy(
            x_hbm.at[at(piece)], own.at[at(piece)], load_sems.at[i]
        )
        load.start()
        return load

    def signal(target):
        pl.semaphore_signal(
            barrier, inc=1, device_id=target, device_id_type=pl.DeviceIdType.LOGICAL
        )

    def round_own(piece):
        own16[at(piece)] = own[at(piece)].astype(jnp.bfloat16)

    def add(got, piece):
        o_ref[at(piece)] = own[at(piece)] + got[at(piece)].astype(jnp.float32)

    def in_strips(src, dst, tiles, target):
        return {t: [remote(src, dst, s, target) for s in _strips(t)] for t in tiles}

    f_in = in_strips(x_hbm, got32, _F_HEAD, _D10) | in_strips(own16, got16, _F_REST, _D10)
    f_on = in_strips(got32, got32, _F_HEAD, _D00) | in_strips(got16, got16, _F_REST, _D00)
    f_tiles = [(got32, t) for t in _F_HEAD] + [(got16, t) for t in _F_REST]
    c_head = [remote(x_hbm, got32, p, _D00) for p in _C_HEAD]
    c_rest = [remote(own16, got16, p, _D00) for p in _C_REST]
    r_early = [remote(own16, got16, p, _D10) for p in _R_EARLY]
    r_late = remote(own16, got16, _R_LATE, _D10)
    g_on = remote(got16, got16, _G, _D10)
    a_low_in = remote(own16, got16, _A_LOW, _D11)
    a_low_on = remote(got16, got16, _A_LOW, _D01)
    a_high_11 = remote(own16, got16, _A_HIGH, _D11)
    a_high_01 = remote(own16, got16, _A_HIGH, _D01)
    assert n_copies == _N_COPIES


    def chip_01():
        signal(_D11)
        pl.semaphore_wait(barrier, 1)
        for copy in c_head:
            copy().start()
        loads = [start_load(i, p) for i, p in enumerate(_C_REST + [_rows(0, 64)])]
        signal(_D00)
        for load, piece, copy in zip(loads, _C_REST, c_rest):
            load.wait()
            round_own(piece)
            copy().start()
        loads[-1].wait()
        for copy in c_head + c_rest:
            copy().wait_send()
        a_low_on().wait_recv()
        add(got16, _A_LOW)
        a_high_01().wait_recv()
        add(got16, _A_HIGH)

    def chip_10():
        signal(_D11)
        signal(_D00)
        start_load(0, _rows(0, 256)).wait()
        round_own(_rows(0, 256))
        pl.semaphore_wait(barrier, 2)
        a_low_in().start()
        a_high_11().start()
        for _, tile in f_tiles:
            for arrived, onward in zip(f_in[tile], f_on[tile]):
                arrived().wait_recv()
                onward().start()
        for got, tile in f_tiles:
            add(got, tile)
        g_on().wait_recv()
        add(got16, _G)
        for _, tile in f_tiles:
            for copy in f_on[tile]:
                copy().wait_send()
        a_low_in().wait_send()
        a_high_11().wait_send()
        for piece, copy in zip(_R_EARLY + [_R_LATE], r_early + [r_late]):
            copy().wait_recv()
            add(got16, piece)

    def chip_11():
        signal(_D10)
        loads = [start_load(i, piece) for i, (piece, _) in enumerate(_F_GROUPS)]
        pl.semaphore_wait(barrier, 2)
        for tile in _F_HEAD:
            for copy in f_in[tile]:
                copy().start()
        late = []
        for load, (piece, tiles) in zip(loads, _F_GROUPS):
            load.wait()
            round_own(piece)
            for tile in tiles:
                for copy in f_in[tile]:
                    copy().start()
            if not late:
                rest = [_rows(56, 120), _R_LATE, _rows(0, 8)]
                late = [start_load(len(loads) + i, p) for i, p in enumerate(rest)]
        late[0].wait()
        round_own(_rows(56, 120))
        for copy in r_early:
            copy().start()
        late[1].wait()
        round_own(_R_LATE)
        r_late().start()
        late[2].wait()
        a_low_in().wait_recv()
        a_low_on().start()
        add(got16, _A_LOW)
        for _, tile in f_tiles:
            for copy in f_in[tile]:
                copy().wait_send()
        for copy in r_early + [r_late, a_low_on]:
            copy().wait_send()
        a_high_11().wait_recv()
        add(got16, _A_HIGH)

    def chip_00():
        signal(_D01)
        signal(_D10)
        start_load(0, _rows(0, 256)).wait()
        round_own(_A_HIGH)
        pl.semaphore_wait(barrier, 2)
        a_high_01().start()
        for piece, copy in zip(_C_HEAD, c_head):
            copy().wait_recv()
            add(got32, piece)
        for i, (piece, copy) in enumerate(zip(_C_REST[:-2], c_rest)):
            copy().wait_recv()
            if i + 1 == _G_READY:
                g_on().start()
            add(got16, piece)
        a_high_01().wait_send()
        g_on().wait_send()

        def wait_tile(tile):
            for copy in f_on[tile]:
                copy().wait_recv()

        for got, tile in f_tiles[:-2]:
            wait_tile(tile)
            add(got, tile)
        c_rest[-2]().wait_recv()
        add(got16, _C_REST[-2])
        wait_tile(_F_REST[-2])
        add(got16, _F_REST[-2])
        wait_tile(_F_REST[-1])
        c_rest[-1]().wait_recv()
        add(got16, _C_REST[-1])
        add(got16, _F_REST[-1])

    me = 2 * lax.axis_index("x") + lax.axis_index("y")
    pl.when(me == _D01)(chip_01)
    pl.when(me == _D10)(chip_10)
    pl.when(me == _D11)(chip_11)
    pl.when(me == _D00)(chip_00)


def pallas_dist_ar_xy_y_m256_n256_kernel(x: jax.Array):
    assert x.shape == (256, 256) and x.dtype == jnp.float32
    return pl.pallas_call(
        _body,
        out_shape=jax.ShapeDtypeStruct(x.shape, x.dtype),
        in_specs=[pl.BlockSpec(memory_space=pltpu.HBM)],
        out_specs=pl.BlockSpec(memory_space=pltpu.VMEM),
        scratch_shapes=[
            pltpu.VMEM(x.shape, jnp.float32),
            pltpu.VMEM(x.shape, jnp.bfloat16),
            pltpu.VMEM(x.shape, jnp.float32),
            pltpu.VMEM(x.shape, jnp.bfloat16),
            pltpu.SemaphoreType.DMA((_N_LOADS,)),
            pltpu.SemaphoreType.DMA((_N_COPIES,)),
            pltpu.SemaphoreType.DMA((_N_COPIES,)),
        ],
        compiler_params=pltpu.CompilerParams(
            collective_id=0,
            disable_semaphore_checks=True,
        ),
    )(x)
```
